```python
import numpy as np

kernel_name = "dist_moe_shared_ep_outshard_n512_d256_e2_h512"

def setup_inputs():
    x = np.random.randn(512, 256).astype(np.float32)
    router_W = np.random.randn(256, 8).astype(np.float32) * 0.1
    scores64 = x.astype(np.float64) @ router_W.astype(np.float64)
    route_idx = np.argsort(-scores64, axis=-1)[:, :1].astype(np.int32)
    expert_W = np.random.randn(8, 256, 512).astype(np.float32) * 0.02
    shared_W = np.random.randn(256, 512).astype(np.float32) * 0.02
    return {"x": x, "router_W": router_W, "route_idx": route_idx, "expert_W": expert_W, "shared_W": shared_W}

def reference(x, router_W, route_idx, expert_W, shared_W):
    scores = x @ router_W
    s_max = scores.max(axis=-1, keepdims=True)
    probs = np.exp(scores - s_max)
    probs = probs / probs.sum(axis=-1, keepdims=True)
    shared = x @ shared_W
    out = np.zeros((512, 512), dtype=np.float32)
    for i in range(512):
        e = int(route_idx[i, 0])
        out[i] = shared[i] + probs[i, e] * (x[i] @ expert_W[e])
    return out
```

```python
import functools

import jax
import jax.numpy as jnp
from jax import lax
from jax.experimental import pallas as pl
from jax.experimental.pallas import tpu as pltpu

N_DEV = 4
N_TOK = 512
D = 256
H = 512
N_EXP = 8
E_LOC = N_EXP // N_DEV
BLK = N_TOK // N_DEV


def _kernel(x_ref, rw_ref, route_ref, ew_ref, sw_ref, out_ref,
            ysend, recv, send_sems, recv_sems):
    my = lax.axis_index("i")

    barrier_sem = pltpu.get_barrier_semaphore()
    for d in range(1, N_DEV):
        pl.semaphore_signal(barrier_sem, inc=1, device_id=((my + d) % N_DEV,),
                            device_id_type=pl.DeviceIdType.MESH)

    w0 = ew_ref[0].astype(jnp.bfloat16)
    w1 = ew_ref[1].astype(jnp.bfloat16)

    def partial_block(k):
        start = pl.multiple_of(k * BLK, BLK)
        xb = x_ref[pl.ds(start, BLK), :].astype(jnp.bfloat16)
        r = route_ref[pl.ds(start, BLK), :]
        m0 = r == (my * E_LOC)
        m1 = r == (my * E_LOC + 1)
        x0 = jnp.where(m0, xb, jnp.zeros_like(xb))
        x1 = jnp.where(m1, xb, jnp.zeros_like(xb))
        y = jnp.dot(x0, w0, preferred_element_type=jnp.float32)
        y = y + jnp.dot(x1, w1, preferred_element_type=jnp.float32)
        return y

    def rdma(d):
        k = (my + d) % N_DEV
        return pltpu.make_async_remote_copy(
            src_ref=ysend.at[d - 1],
            dst_ref=recv.at[d - 1],
            send_sem=send_sems.at[d - 1],
            recv_sem=recv_sems.at[d - 1],
            device_id=(k,),
            device_id_type=pl.DeviceIdType.MESH,
        )

    first = True
    for d in range(1, N_DEV):
        k = (my + d) % N_DEV
        ysend[d - 1] = partial_block(k).astype(jnp.bfloat16)
        if first:
            pl.semaphore_wait(barrier_sem, N_DEV - 1)
            first = False
        rdma(d).start()

    own = partial_block(my)
    start = pl.multiple_of(my * BLK, BLK)
    xf = x_ref[pl.ds(start, BLK), :]
    xb = xf.astype(jnp.bfloat16)
    shared = jnp.dot(xb, sw_ref[...].astype(jnp.bfloat16),
                     preferred_element_type=jnp.float32)
    scores = jnp.dot(xf, rw_ref[...], preferred_element_type=jnp.float32,
                     precision=lax.Precision.HIGHEST)
    smax = jnp.max(scores, axis=-1, keepdims=True)
    p = jnp.exp(scores - smax)
    denom = jnp.sum(p, axis=-1, keepdims=True)
    r = route_ref[pl.ds(start, BLK), :]
    lane = lax.broadcasted_iota(jnp.int32, scores.shape, 1)
    psel = jnp.sum(jnp.where(lane == r, p, 0.0), axis=-1, keepdims=True)
    gate = psel / denom

    acc = own
    for d in range(1, N_DEV):
        rdma(d).wait()
        acc = acc + recv[d - 1].astype(jnp.float32)
    out_ref[...] = shared + gate * acc


def pallas_dist_moe_shared_ep_outshard_n512_d256_e2_h512_kernel(
    x, router_W, route_idx, expert_W, shared_W,
):
    vmem = pl.BlockSpec(memory_space=pltpu.VMEM)
    return pl.pallas_call(
        _kernel,
        out_shape=jax.ShapeDtypeStruct((BLK, H), jnp.float32),
        in_specs=[vmem, vmem, vmem, vmem, vmem],
        out_specs=vmem,
        scratch_shapes=[
            pltpu.VMEM((N_DEV - 1, BLK, H), jnp.bfloat16),
            pltpu.VMEM((N_DEV - 1, BLK, H), jnp.bfloat16),
            pltpu.SemaphoreType.DMA((N_DEV - 1,)),
            pltpu.SemaphoreType.DMA((N_DEV - 1,)),
        ],
        compiler_params=pltpu.CompilerParams(collective_id=0),
    )(x, router_W, route_idx, expert_W, shared_W)
```

```python
import jax
import jax.numpy as jnp
from jax import lax
from jax.experimental import pallas as pl
from jax.experimental.pallas import tpu as pltpu

N_DEV = 4
N_TOK = 512
D = 256
H = 512
N_EXP = 8
E_LOC = N_EXP // N_DEV
BLK = N_TOK // N_DEV
NCH = 2
CW = H // NCH
PIECE = 16
SIZES = tuple(range(PIECE, BLK + 1, PIECE))
NTILE = N_TOK // BLK
BF16 = jnp.bfloat16
F32 = jnp.float32


def _lane_incl_prefix(v):
    lane = lax.broadcasted_iota(jnp.int32, v.shape, 1)
    s = 1
    while s < v.shape[1]:
        v = v + jnp.where(lane >= s, pltpu.roll(v, s, 1), jnp.zeros_like(v))
        s *= 2
    return v


def _pick(vals, idx):
    out = vals[0]
    for i in range(1, len(vals)):
        out = jnp.where(idx == i, vals[i], out)
    return out


def _round_up(v, m):
    return ((v + (m - 1)) // m) * m


def _kernel(x_hbm, rwT_hbm, route_hbm, ew_hbm, sw_hbm, out_ref,
            xv, rwv, rtv, ewv, swv, xgv, yv, rv, qv,
            in_sems, send_sems, recv_sems):
    my = lax.axis_index("i")

    barrier_sem = pltpu.get_barrier_semaphore()
    for d in range(1, N_DEV):
        pl.semaphore_signal(barrier_sem, inc=1, device_id=((my + d) % N_DEV,),
                            device_id_type=pl.DeviceIdType.MESH)
    c_route = pltpu.make_async_copy(route_hbm, rtv, in_sems.at[0])
    c_rw = pltpu.make_async_copy(rwT_hbm, rwv, in_sems.at[1])
    c_sw = pltpu.make_async_copy(sw_hbm, swv, in_sems.at[2])
    c_x = [pltpu.make_async_copy(x_hbm.at[pl.ds(k * BLK, BLK)], xv.at[pl.ds(k * BLK, BLK)],
                                 in_sems.at[3 + k]) for k in range(N_DEV)]
    c_w = [pltpu.make_async_copy(ew_hbm.at[:, :, pl.ds(c * CW, CW)], ewv.at[c],
                                 in_sems.at[3 + N_DEV + c]) for c in range(NCH)]
    for cp in [c_route, c_rw] + c_x + c_w:
        cp.start()

    sub = lax.broadcasted_iota(jnp.int32, (BLK, BLK), 0)

    c_route.wait()
    route = rtv[...]
    r4 = jnp.concatenate([route[:, k * BLK:(k + 1) * BLK] for k in range(N_DEV)], axis=0)
    m4 = ((r4 >> 1) == my).astype(jnp.int32)
    incl4 = _lane_incl_prefix(m4)
    pos4 = incl4 - m4
    neg = jnp.full(r4.shape, -1, jnp.int32)
    code0 = jnp.where(r4 == my * E_LOC, pos4, neg)
    code1 = jnp.where(r4 == my * E_LOC + 1, pos4, neg)
    cnt = [incl4[k, BLK - 1] for k in range(N_DEV)]
    seg = [_round_up(c, PIECE) for c in cnt]
    size = [jnp.maximum(s, PIECE) for s in seg]
    base = [jnp.int32(0)]
    for k in range(1, N_DEV):
        base.append(base[k - 1] + seg[k - 1])
    total = base[N_DEV - 1] + seg[N_DEV - 1]
    ntiles = jnp.minimum((total + PIECE + (BLK - 1)) // BLK, NTILE)

    for k in range(N_DEV):
        g0 = jnp.where(sub == jnp.broadcast_to(code0[k:k + 1, :], (BLK, BLK)), 1.0, 0.0).astype(BF16)
        g1 = jnp.where(sub == jnp.broadcast_to(code1[k:k + 1, :], (BLK, BLK)), 1.0, 0.0).astype(BF16)
        c_x[k].wait()
        xb = xv[pl.ds(k * BLK, BLK), :].astype(BF16)
        bk = pl.multiple_of(base[k], PIECE)
        xgv[pl.ds(bk, BLK), 0:D] = jnp.dot(g0, xb, preferred_element_type=F32).astype(BF16)
        xgv[pl.ds(bk, BLK), D:2 * D] = jnp.dot(g1, xb, preferred_element_type=F32).astype(BF16)
    tail = pl.multiple_of(base[N_DEV - 1] + BLK, PIECE)
    xgv[pl.ds(tail, BLK), :] = jnp.zeros((BLK, E_LOC * D), BF16)

    def chunk_send(d, k, s, c):
        return pltpu.make_async_remote_copy(
            src_ref=yv.at[pl.ds(pl.multiple_of(_pick(base, k), PIECE), s), pl.ds(c * CW, CW)],
            dst_ref=rv.at[my, pl.ds(0, s), pl.ds(c * CW, CW)],
            send_sem=send_sems.at[d - 1],
            recv_sem=recv_sems.at[my],
            device_id=(k,),
            device_id_type=pl.DeviceIdType.MESH,
        )

    def total_desc(slot_send, slot_recv, s):
        return pltpu.make_async_remote_copy(
            src_ref=yv.at[pl.ds(0, s)],
            dst_ref=rv.at[slot_recv, pl.ds(0, s)],
            send_sem=send_sems.at[slot_send],
            recv_sem=recv_sems.at[slot_recv],
            device_id=(slot_recv,),
            device_id_type=pl.DeviceIdType.MESH,
        )

    size_to = [_pick(size, (my + d) % N_DEV) for d in range(1, N_DEV)]

    for c in range(NCH):
        c_w[c].wait()
        if c == NCH - 1:
            c_sw.start()
        wc = ewv[c].reshape(E_LOC * D, CW).astype(BF16)
        for t in range(NTILE):
            @pl.when(t < ntiles)
            def _():
                yt = jnp.dot(xgv[t * BLK:(t + 1) * BLK, :], wc, preferred_element_type=F32)
                yv[t * BLK:(t + 1) * BLK, c * CW:(c + 1) * CW] = yt.astype(BF16)
        if c == 0:
            pl.semaphore_wait(barrier_sem, N_DEV - 1)
        for d in range(1, N_DEV):
            k = (my + d) % N_DEV
            for s in SIZES:
                @pl.when(size_to[d - 1] == s)
                def _():
                    chunk_send(d, k, s, c).start()

    r_me = _pick([r4[k:k + 1, :] for k in range(N_DEV)], my)
    sub8 = lax.broadcasted_iota(jnp.int32, (8, BLK), 0)
    m_me = (sub8 == (r_me >> 1)).astype(jnp.int32)
    incl_me = _lane_incl_prefix(m_me)
    code_me = jnp.where(m_me > 0, incl_me - m_me, jnp.full(m_me.shape, -1, jnp.int32))
    recv_size = [jnp.maximum(_round_up(incl_me[j, BLK - 1], PIECE), PIECE) for j in range(N_DEV)]
    own_seg = _round_up(_pick([incl_me[j, BLK - 1] for j in range(N_DEV)], my), PIECE)

    kk = pl.multiple_of(my * BLK, BLK)
    xf = xv[pl.ds(kk, BLK), :]
    c_rw.wait()
    scT = lax.dot_general(rwv[...], xf, (((1,), (1,)), ((), ())),
                          preferred_element_type=F32,
                          precision=lax.Precision.HIGHEST)
    smax = jnp.max(scT, axis=0, keepdims=True)
    pe = jnp.exp(scT - smax)
    denom = jnp.sum(pe, axis=0, keepdims=True)
    esub = lax.broadcasted_iota(jnp.int32, scT.shape, 0)
    psel = jnp.sum(jnp.where(esub == r_me, pe, 0.0), axis=0, keepdims=True)
    gate_b = jnp.broadcast_to(psel / denom, (BLK, BLK))
    for j in range(N_DEV):
        hit = sub == jnp.broadcast_to(code_me[j:j + 1, :], (BLK, BLK))
        qv[j] = jnp.where(hit, gate_b, 0.0).astype(BF16)

    c_sw.wait()
    out_ref[...] = jnp.dot(xf.astype(BF16), swv[...].astype(BF16), preferred_element_type=F32)

    base_my = pl.multiple_of(_pick(base, my), PIECE)
    for s in SIZES:
        @pl.when(own_seg == s)
        def _():
            out_ref[...] += lax.dot_general(
                qv[my, 0:s, :], yv[pl.ds(base_my, s), :], (((0,), (0,)), ((), ())),
                preferred_element_type=F32)

    for d in range(1, N_DEV):
        j = (my - d) % N_DEV
        rs = _pick(recv_size, j)
        for s in SIZES:
            @pl.when(rs == s)
            def _():
                total_desc(0, j, s).wait_recv()
                out_ref[...] += lax.dot_general(
                    qv[j, 0:s, :], rv[j, 0:s, :], (((0,), (0,)), ((), ())),
                    preferred_element_type=F32)

    for d in range(1, N_DEV):
        for s in SIZES:
            @pl.when(size_to[d - 1] == s)
            def _():
                total_desc(d - 1, 0, s).wait_send()


def pallas_dist_moe_shared_ep_outshard_n512_d256_e2_h512_kernel(
    x, router_W, route_idx, expert_W, shared_W,
):
    anyspec = pl.BlockSpec(memory_space=pl.ANY)
    return pl.pallas_call(
        _kernel,
        out_shape=jax.ShapeDtypeStruct((BLK, H), F32),
        in_specs=[anyspec] * 5,
        out_specs=pl.BlockSpec(memory_space=pltpu.VMEM),
        scratch_shapes=[
            pltpu.VMEM((N_TOK, D), F32),
            pltpu.VMEM((N_EXP, D), F32),
            pltpu.VMEM((1, N_TOK), jnp.int32),
            pltpu.VMEM((NCH, E_LOC, D, CW), F32),
            pltpu.VMEM((D, H), F32),
            pltpu.VMEM((N_TOK + BLK, E_LOC * D), BF16),
            pltpu.VMEM((N_TOK, H), BF16),
            pltpu.VMEM((N_DEV, BLK, H), BF16),
            pltpu.VMEM((N_DEV, BLK, BLK), BF16),
            pltpu.SemaphoreType.DMA((3 + N_DEV + NCH,)),
            pltpu.SemaphoreType.DMA((N_DEV - 1,)),
            pltpu.SemaphoreType.DMA((N_DEV,)),
        ],
        compiler_params=pltpu.CompilerParams(collective_id=0),
    )(x, router_W.T, route_idx.reshape(1, N_TOK), expert_W, shared_W)
```

```python
import jax
import jax.numpy as jnp
from jax import lax
from jax.experimental import pallas as pl
from jax.experimental.pallas import tpu as pltpu

N_DEV = 4
N_TOK = 512
D = 256
H = 512
N_EXP = 8
E_LOC = N_EXP // N_DEV
BLK = N_TOK // N_DEV
NCH = 2
CW = H // NCH
PIECE = 16
SIZES = tuple(range(PIECE, BLK + 1, PIECE))
NTILE = N_TOK // BLK
GHALF = BLK // 2
ZROWS = BLK + 2 * PIECE
BF16 = jnp.bfloat16
F32 = jnp.float32


def _lane_incl_prefix(mask_bool, tri):
    mf = jnp.where(mask_bool, 1.0, 0.0).astype(BF16)
    return jnp.dot(mf, tri, preferred_element_type=F32).astype(jnp.int32)


def _pick(vals, idx):
    out = vals[0]
    for i in range(1, len(vals)):
        out = jnp.where(idx == i, vals[i], out)
    return out


def _round_up(v, m):
    return ((v + (m - 1)) // m) * m


def _kernel(x_hbm, rwT_hbm, route_hbm, ew_hbm, sw_hbm, out_ref,
            xv, rwv, rtv, ewv, swv, xgv, yv, rv, qv,
            in_sems, send_sems, recv_sems):
    my = lax.axis_index("i")

    barrier_sem = pltpu.get_barrier_semaphore()
    for d in range(1, N_DEV):
        pl.semaphore_signal(barrier_sem, inc=1, device_id=((my + d) % N_DEV,),
                            device_id_type=pl.DeviceIdType.MESH)
    c_route = pltpu.make_async_copy(route_hbm, rtv, in_sems.at[0])
    c_rw = pltpu.make_async_copy(rwT_hbm, rwv, in_sems.at[1])
    c_sw = pltpu.make_async_copy(sw_hbm, swv, in_sems.at[2])
    c_x = [pltpu.make_async_copy(x_hbm.at[pl.ds(k * BLK, BLK)], xv.at[pl.ds(k * BLK, BLK)],
                                 in_sems.at[3 + k]) for k in range(N_DEV)]
    c_w = [pltpu.make_async_copy(ew_hbm.at[:, :, pl.ds(c * CW, CW)], ewv.at[c],
                                 in_sems.at[3 + N_DEV + c]) for c in range(NCH)]
    for cp in [c_route, c_rw] + c_x + c_w:
        cp.start()

    sub = lax.broadcasted_iota(jnp.int32, (BLK, BLK), 0)
    lane = lax.broadcasted_iota(jnp.int32, (BLK, BLK), 1)
    tri = jnp.where(sub <= lane, 1.0, 0.0).astype(BF16)

    c_route.wait()
    route = rtv[...]
    r4 = jnp.concatenate([route[:, k * BLK:(k + 1) * BLK] for k in range(N_DEV)], axis=0)
    mb4 = (r4 >> 1) == my
    incl4 = _lane_incl_prefix(mb4, tri)
    pos4 = incl4 - mb4.astype(jnp.int32)
    neg = jnp.full(r4.shape, -1, jnp.int32)
    code0 = jnp.where(r4 == my * E_LOC, pos4, neg)
    code1 = jnp.where(r4 == my * E_LOC + 1, pos4, neg)
    cnt = [incl4[k, BLK - 1] for k in range(N_DEV)]
    seg = [_round_up(c, PIECE) for c in cnt]
    size = [jnp.maximum(s, PIECE) for s in seg]
    base = [jnp.int32(0)]
    for k in range(1, N_DEV):
        base.append(base[k - 1] + seg[k - 1])
    total = base[N_DEV - 1] + seg[N_DEV - 1]
    ntiles = jnp.minimum((total + PIECE + (BLK - 1)) // BLK, NTILE)

    wid = []
    for k in range(N_DEV):
        c_x[k].wait()
        xb = xv[pl.ds(k * BLK, BLK), :].astype(BF16)
        bk = pl.multiple_of(base[k], PIECE)
        half = cnt[k] <= GHALF
        wid.append(jnp.where(half, GHALF, BLK))
        for S in (GHALF, BLK):
            @pl.when(half if S == GHALF else jnp.logical_not(half))
            def _():
                subs = lax.broadcasted_iota(jnp.int32, (S, BLK), 0)
                g0 = jnp.where(subs == jnp.broadcast_to(code0[k:k + 1, :], (S, BLK)), 1.0, 0.0)
                g1 = jnp.where(subs == jnp.broadcast_to(code1[k:k + 1, :], (S, BLK)), 1.0, 0.0)
                g = jnp.concatenate([g0, g1], axis=0).astype(BF16)
                xg = jnp.dot(g, xb, preferred_element_type=F32).astype(BF16)
                xgv[pl.ds(bk, S), 0:D] = xg[0:S]
                xgv[pl.ds(bk, S), D:2 * D] = xg[S:2 * S]
    tail = pl.multiple_of(base[N_DEV - 1] + wid[N_DEV - 1], PIECE)
    xgv[pl.ds(tail, ZROWS), :] = jnp.zeros((ZROWS, E_LOC * D), BF16)

    def chunk_send(d, k, s, c):
        return pltpu.make_async_remote_copy(
            src_ref=yv.at[pl.ds(pl.multiple_of(_pick(base, k), PIECE), s), pl.ds(c * CW, CW)],
            dst_ref=rv.at[my, pl.ds(0, s), pl.ds(c * CW, CW)],
            send_sem=send_sems.at[d - 1],
            recv_sem=recv_sems.at[my],
            device_id=(k,),
            device_id_type=pl.DeviceIdType.MESH,
        )

    def total_desc(slot_send, slot_recv, s):
        return pltpu.make_async_remote_copy(
            src_ref=yv.at[pl.ds(0, s)],
            dst_ref=rv.at[slot_recv, pl.ds(0, s)],
            send_sem=send_sems.at[slot_send],
            recv_sem=recv_sems.at[slot_recv],
            device_id=(slot_recv,),
            device_id_type=pl.DeviceIdType.MESH,
        )

    size_to = [_pick(size, (my + d) % N_DEV) for d in range(1, N_DEV)]

    for c in range(NCH):
        c_w[c].wait()
        if c == NCH - 1:
            c_sw.start()
        wc = ewv[c].reshape(E_LOC * D, CW).astype(BF16)
        for n in range(1, NTILE + 1):
            @pl.when(ntiles == n)
            def _():
                yt = jnp.dot(xgv[0:n * BLK, :], wc, preferred_element_type=F32)
                yv[0:n * BLK, c * CW:(c + 1) * CW] = yt.astype(BF16)
        if c == 0:
            pl.semaphore_wait(barrier_sem, N_DEV - 1)
        for d in range(1, N_DEV):
            k = (my + d) % N_DEV
            for s in SIZES:
                @pl.when(size_to[d - 1] == s)
                def _():
                    chunk_send(d, k, s, c).start()

    r_me = _pick([r4[k:k + 1, :] for k in range(N_DEV)], my)
    sub8 = lax.broadcasted_iota(jnp.int32, (8, BLK), 0)
    mb_me = sub8 == (r_me >> 1)
    incl_me = _lane_incl_prefix(mb_me, tri)
    code_me = jnp.where(mb_me, incl_me - 1, jnp.full(incl_me.shape, -1, jnp.int32))
    recv_size = [jnp.maximum(_round_up(incl_me[j, BLK - 1], PIECE), PIECE) for j in range(N_DEV)]
    own_seg = _round_up(_pick([incl_me[j, BLK - 1] for j in range(N_DEV)], my), PIECE)

    kk = pl.multiple_of(my * BLK, BLK)
    xf = xv[pl.ds(kk, BLK), :]
    c_rw.wait()
    scT = lax.dot_general(rwv[...], xf, (((1,), (1,)), ((), ())),
                          preferred_element_type=F32,
                          precision=lax.Precision.HIGHEST)
    smax = jnp.max(scT, axis=0, keepdims=True)
    pe = jnp.exp(scT - smax)
    denom = jnp.sum(pe, axis=0, keepdims=True)
    esub = lax.broadcasted_iota(jnp.int32, scT.shape, 0)
    psel = jnp.sum(jnp.where(esub == r_me, pe, 0.0), axis=0, keepdims=True)
    gate_b = jnp.broadcast_to(psel / denom, (BLK, BLK))
    for j in range(N_DEV):
        hit = sub == jnp.broadcast_to(code_me[j:j + 1, :], (BLK, BLK))
        qv[j] = jnp.where(hit, gate_b, 0.0).astype(BF16)

    c_sw.wait()
    out_ref[...] = jnp.dot(xf.astype(BF16), swv[...].astype(BF16), preferred_element_type=F32)

    base_my = pl.multiple_of(_pick(base, my), PIECE)
    for s in SIZES:
        @pl.when(own_seg == s)
        def _():
            out_ref[...] += lax.dot_general(
                qv[my, 0:s, :], yv[pl.ds(base_my, s), :], (((0,), (0,)), ((), ())),
                preferred_element_type=F32)

    for d in range(1, N_DEV):
        j = (my - d) % N_DEV
        rs = _pick(recv_size, j)
        for s in SIZES:
            @pl.when(rs == s)
            def _():
                total_desc(0, j, s).wait_recv()
                out_ref[...] += lax.dot_general(
                    qv[j, 0:s, :], rv[j, 0:s, :], (((0,), (0,)), ((), ())),
                    preferred_element_type=F32)

    for d in range(1, N_DEV):
        for s in SIZES:
            @pl.when(size_to[d - 1] == s)
            def _():
                total_desc(d - 1, 0, s).wait_send()


def pallas_dist_moe_shared_ep_outshard_n512_d256_e2_h512_kernel(
    x, router_W, route_idx, expert_W, shared_W,
):
    anyspec = pl.BlockSpec(memory_space=pl.ANY)
    return pl.pallas_call(
        _kernel,
        out_shape=jax.ShapeDtypeStruct((BLK, H), F32),
        in_specs=[anyspec] * 5,
        out_specs=pl.BlockSpec(memory_space=pltpu.VMEM),
        scratch_shapes=[
            pltpu.VMEM((N_TOK, D), F32),
            pltpu.VMEM((N_EXP, D), F32),
            pltpu.VMEM((1, N_TOK), jnp.int32),
            pltpu.VMEM((NCH, E_LOC, D, CW), F32),
            pltpu.VMEM((D, H), F32),
            pltpu.VMEM((N_TOK + ZROWS, E_LOC * D), BF16),
            pltpu.VMEM((N_TOK, H), BF16),
            pltpu.VMEM((N_DEV, BLK, H), BF16),
            pltpu.VMEM((N_DEV, BLK, BLK), BF16),
            pltpu.SemaphoreType.DMA((3 + N_DEV + NCH,)),
            pltpu.SemaphoreType.DMA((N_DEV - 1,)),
            pltpu.SemaphoreType.DMA((N_DEV,)),
        ],
        compiler_params=pltpu.CompilerParams(collective_id=0),
    )(x, router_W.T, route_idx.reshape(1, N_TOK), expert_W, shared_W)
```
